```python
import numpy as np

kernel_name = "dist_sparse_attn_strided_qseq_b1_sq1024_skv1024_hq8_dh128"

def setup_inputs():
    x = np.random.randn(1, 4096, 1024).astype(np.float32)
    Wq = np.random.randn(1024, 4096).astype(np.float32) * 0.02
    K_ext = np.random.randn(1, 1024, 32, 128).astype(np.float32)
    V_ext = np.random.randn(1, 1024, 32, 128).astype(np.float32)
    Wo = np.random.randn(4096, 1024).astype(np.float32) * 0.02
    return {"x": x, "Wq": Wq, "K_ext": K_ext, "V_ext": V_ext, "Wo": Wo}

def reference(x, Wq, K_ext, V_ext, Wo):
    B, Sq, Skv, Hq, Dh = 1, 4096, 1024, 32, 128
    Q = (x @ Wq).reshape(B, Sq, Hq, Dh)
    qb = (np.arange(Sq) // 64)[:, None]
    kb = (np.arange(Skv) // 64)[None, :]
    mask = (qb == kb) | ((kb % 4) == (qb % 4))
    scores = np.einsum('bihd,bjhd->bhij', Q, K_ext).astype(np.float32) * 0.08838834764831843
    scores = np.where(mask[None, None, :, :], scores, -1e9)
    scores_max = scores.max(axis=-1, keepdims=True)
    w = np.exp(scores - scores_max)
    row_keep = mask.any(axis=1)
    w_sum = np.where(row_keep[None, None, :, None], w.sum(axis=-1, keepdims=True), 1.0)
    w = w / w_sum
    w = np.where(row_keep[None, None, :, None], w, 0.0)
    ctx = np.einsum('bhij,bjhd->bihd', w, V_ext).reshape(B, Sq, Hq * Dh)
    return ctx @ Wo
```

```python
import os
import jax
import jax.numpy as jnp
from jax import lax
from jax.experimental import pallas as pl
from jax.experimental.pallas import tpu as pltpu

E = os.environ.get
NOCOMM = int(E("NOCOMM", 0))
LOOK = int(E("LOOK", 2))
BAR = int(E("BAR", 1))
CW = int(E("CW", 256))
OM = int(E("OM", 512))
SCOPES = int(E("SCOPES", 0))
KC = 128
NKC = 1024 // KC
NJ = 1024 // CW
F32, BF16 = jnp.float32, jnp.bfloat16
QSCALE = 0.08838834764831843 * 1.4426950408889634


def _merge(*jobs):
    keyed = [((i + 0.5) / len(js), n, i, j) for n, js in enumerate(jobs) for i, j in enumerate(js)]
    return [j for _, _, _, j in sorted(keyed, key=lambda t: t[:3])]


def _body(x_hbm, wq_hbm, k_hbm, v_hbm, wo_hbm, out_hbm,
          xf, wqf, wof, kf, vf, xb, wqb, wob, kb, vb, qb, cb, acc, sbuf, rbuf,
          x_sem, wq_sem, wo_sem, kv_sem, out_sem, tx_x, rx_x, tx_q, rx_q, tx_o, rx_o, tx_p, rx_p):
    me = lax.axis_index("i")
    row_peer = me ^ 1
    head_peer = 3 - me
    mesh_id = pl.DeviceIdType.MESH

    if not NOCOMM:
        barrier = pltpu.get_barrier_semaphore()
        for peer in (row_peer, head_peer):
            pl.semaphore_signal(barrier, inc=1, device_id=(peer,), device_id_type=mesh_id)

    def remote(src, dst, tx, rx, peer):
        return pltpu.make_async_remote_copy(src, dst, tx, rx, device_id=(peer,), device_id_type=mesh_id)

    def x_load(kc):
        c = pl.ds(kc * KC, KC)
        return pltpu.make_async_copy(x_hbm.at[0, :, c], xf.at[:, c], x_sem.at[kc])

    def wq_load(kc):
        r = pl.ds(kc * KC, KC)
        return pltpu.make_async_copy(wq_hbm.at[r, :], wqf.at[r, :], wq_sem.at[kc])

    def wo_load():
        return pltpu.make_async_copy(wo_hbm, wof, wo_sem)

    def kv_start(g, m):
        head0 = (me if g == 0 else head_peer) * 8
        for t, (src, dst) in enumerate(((k_hbm, kf), (v_hbm, vf))):
            for h in range(8):
                pltpu.make_async_copy(src.at[:, m, :, head0 + h, :], dst.at[g, m, h], kv_sem.at[t, g, m]).start()

    def kv_wait(g, m):
        for t, dst in enumerate((kf, vf)):
            pltpu.make_async_copy(dst.at[g, m], dst.at[g, m], kv_sem.at[t, g, m]).wait()

    def kv_cast(g, m):
        def job(h):
            def run():
                kb[g, m, h] = kf[g, m, h].reshape(256, 128).astype(BF16)
                vb[g, m, h] = vf[g, m, h].reshape(256, 128).astype(BF16)
            return run
        return [job(h) for h in range(8)]

    def wo_cast():
        def job(j):
            def run():
                wob[0, j] = wof[:, j * CW:(j + 1) * CW].astype(BF16)
            return run
        return [job(j) for j in range(NJ)]

    def send_x(m, c=slice(None)):
        return remote(xb.at[0, m, :, c], xb.at[1, m, :, c], tx_x.at[m], rx_x.at[m], row_peer)

    def send_wq(j, r=slice(None)):
        return remote(wqb.at[0, j, r, :], wqb.at[1, j, r, :], tx_q.at[j], rx_q.at[j], head_peer)

    def send_wo(j):
        return remote(wob.at[0, j], wob.at[1, j], tx_o.at[j], rx_o.at[j], head_peer)

    def send_part(j):
        return remote(sbuf.at[j], rbuf.at[j], tx_p.at[j], rx_p.at[j], row_peer)

    def start(cp):
        if not NOCOMM:
            cp.start()

    def recv(cp):
        if not NOCOMM:
            cp.wait_recv()

    def q_proj(items):
        def job(s, m, g, j):
            def run():
                q = jnp.dot(xb[s, m], wqb[g, j], preferred_element_type=F32)
                c0 = g * 1024 + j * 256
                qb[s, m * 256:(m + 1) * 256, c0:c0 + 256] = q.astype(BF16)
            return run
        return [job(*it) for it in items]

    def attn(pairs):
        items = [(s, m, g, 2 * j + i) for s, m, g, j in pairs for i in range(2)]
        live = {}

        def scores(n):
            s, m, g, h = items[n]

            def run():
                c0 = g * 1024 + h * 128
                q = qb[s, m * 256:(m + 1) * 256, c0:c0 + 128]
                sc = lax.dot_general(q, kb[g, m, h], (((1,), (1,)), ((), ())), preferred_element_type=F32)
                p = jnp.exp2(sc - jnp.max(sc, axis=1, keepdims=True))
                live[n] = (p.astype(BF16), jnp.sum(p, axis=1, keepdims=True))
            return run

        def context(n):
            s, m, g, h = items[n]

            def run():
                p, l = live.pop(n)
                c0 = g * 1024 + h * 128
                o = jnp.dot(p, vb[g, m, h], preferred_element_type=F32)
                cb[s, m * 256:(m + 1) * 256, c0:c0 + 128] = (o * pl.reciprocal(l, approx=True)).astype(BF16)
            return run

        jobs = []
        for n in range(len(items) + LOOK):
            if n < len(items):
                jobs.append(scores(n))
            if n >= LOOK:
                jobs.append(context(n - LOOK))
        return jobs

    def o_dot(s, r, g, j):
        return jnp.dot(cb[s, r, g * 1024:(g + 1) * 1024], wob[g, j], preferred_element_type=F32)

    def rows(i):
        return slice(i * OM, (i + 1) * OM)

    def cols(j):
        return slice(j * CW, (j + 1) * CW)

    def o_first(s, j):
        def job(i):
            def run():
                acc[s, rows(i), cols(j)] = o_dot(s, rows(i), 0, j)
            return run
        return [job(i) for i in range(1024 // OM)]

    def o_peer(j, pre):
        def job(i):
            def run():
                base = acc[1, rows(i), cols(j)] if pre else o_dot(1, rows(i), 0, j)
                sbuf[j, rows(i), :] = (base + o_dot(1, rows(i), 1, j)).astype(BF16)
            return run
        return [job(i) for i in range(1024 // OM)]

    def o_own(j, pre):
        def job(i):
            def run():
                base = acc[0, rows(i), cols(j)] if pre else o_dot(0, rows(i), 0, j)
                y = base + o_dot(0, rows(i), 1, j) + rbuf[j, rows(i), :].astype(F32)
                for b in range(OM // 64):
                    m, a = divmod(i * (OM // 64) + b, 4)
                    xf[(4 * a + m) * 64:(4 * a + m + 1) * 64, cols(j)] = y[b * 64:(b + 1) * 64]
            return run
        return [job(i) for i in range(1024 // OM)]

    def out_store(j):
        c = pl.ds(j * CW, CW)
        return pltpu.make_async_copy(xf.at[:, c], out_hbm.at[0, :, c], out_sem.at[j])

    n_scope = [0]

    def run(*jobs):
        def go():
            for job in _merge(*jobs):
                job()
        if SCOPES:
            n_scope[0] += 1
            with jax.named_scope(f"z_{n_scope[0]:02d}"):
                go()
        else:
            go()

    AHEAD = 3
    for kc in range(AHEAD):
        x_load(kc).start()
        wq_load(kc).start()
    for kc in range(NKC):
        c = slice(kc * KC, (kc + 1) * KC)
        x_load(kc).wait()
        wq_load(kc).wait()
        if kc + AHEAD < NKC:
            x_load(kc + AHEAD).start()
            wq_load(kc + AHEAD).start()
        elif kc + AHEAD - NKC < 4:
            kv_start(0, kc + AHEAD - NKC)
        for b in range(16):
            a, m = divmod(b, 4)
            xb[0, m, a * 64:(a + 1) * 64, c] = xf[b * 64:(b + 1) * 64, c].astype(BF16)
        for j in range(4):
            wqb[0, j, c, :] = (wqf[c, j * 256:(j + 1) * 256] * QSCALE).astype(BF16)
        if kc == BAR and not NOCOMM:
            pl.semaphore_wait(barrier, 2)
        if kc >= BAR:
            piece = pl.ds(0, (kc + 1) * KC) if kc == BAR else pl.ds(kc * KC, KC)
            start(send_x(0, piece))
            start(send_wq(0, piece))

        def job(m, j, kc=kc, c=c):
            def go():
                r, cc = slice(m * 512, (m + 1) * 512), slice(j * 256, (j + 1) * 256)
                y = jnp.dot(xb[0, 2 * m:2 * m + 2, :, c].reshape(512, KC), wqb[0, j, c, :], preferred_element_type=F32)
                if kc > 0:
                    y = y + acc[0, r, cc]
                if kc < NKC - 1:
                    acc[0, r, cc] = y
                else:
                    qb[0, r, cc] = y.astype(BF16)
            return go
        run([job(m, j) for j in range(4) for m in range(2)])
    for t in range(1, 4):
        start(send_x(t))
        start(send_wq(t))
    for m in range(AHEAD, 4):
        kv_start(0, m)

    all4 = range(4)
    kv_wait(0, 0)
    run(kv_cast(0, 0))
    run(attn([(0, 0, 0, j) for j in all4]))
    wo_load().start()
    kv_wait(0, 1)
    recv(send_x(0))
    run(kv_cast(0, 1))
    run(q_proj([(1, 0, 0, j) for j in all4]), attn([(0, 1, 0, j) for j in all4]))
    kv_start(1, 0)
    kv_start(1, 1)
    kv_wait(0, 2)
    recv(send_wq(0))
    run(kv_cast(0, 2))
    run(q_proj([(1, 0, 1, 0)] + [(0, m, 1, 0) for m in all4]),
        attn([(1, 0, 0, j) for j in all4] + [(0, 2, 0, j) for j in all4]))
    kv_start(1, 2)
    kv_start(1, 3)
    kv_wait(0, 3)
    wo_load().wait()
    recv(send_x(1))
    recv(send_wq(1))
    run(kv_cast(0, 3))
    run(q_proj([(1, 1, 0, j) for j in all4]), attn([(0, 3, 0, j) for j in all4]), wo_cast())
    kv_wait(1, 0)
    kv_wait(1, 1)
    run(q_proj([(1, 1, 1, 0), (1, 0, 1, 1), (1, 1, 1, 1)]), attn([(1, 1, 0, j) for j in all4]),
        kv_cast(1, 0) + kv_cast(1, 1))
    run(q_proj([(0, m, 1, 1) for m in all4]), attn([(1, m, 1, j) for m in (0, 1) for j in (0, 1)]))
    kv_wait(1, 2)
    kv_wait(1, 3)
    recv(send_x(2))
    recv(send_wq(2))
    for j in range(NJ):
        start(send_wo(j))
    run(q_proj([(1, 2, 0, j) for j in all4]), attn([(0, m, 1, j) for m in (0, 1) for j in (0, 1)]),
        kv_cast(1, 2) + kv_cast(1, 3))
    new2 = [(1, 2, 1, 0), (1, 2, 1, 1), (1, 0, 1, 2), (1, 1, 1, 2), (1, 2, 1, 2)]
    run(_merge(q_proj(new2), attn([(1, 2, 0, j) for j in all4])) + attn(new2))
    recv(send_x(3))
    recv(send_wq(3))
    new3 = [(1, m, 1, 3) for m in range(3)] + [(1, 3, 1, j) for j in all4]
    run(q_proj([(1, 3, 0, j) for j in all4]) + _merge(q_proj(new3), attn([(1, 3, 0, j) for j in all4])))
    run(o_first(1, 0), attn(new3))
    own2 = [(0, m, 1, j) for m in (2, 3) for j in (0, 1)]
    q2, q3 = [(0, m, 1, 2) for m in all4], [(0, m, 1, 3) for m in all4]
    fill = [[q_proj(q2), attn(own2)], [q_proj(q3), attn(q2)], [o_first(0, 0), attn(q3)]]
    for j in range(NJ):
        recv(send_wo(j))
        run(o_peer(j, j == 0))
        start(send_part(j))
        if j * 4 % NJ == 0 and j * 4 // NJ < 3:
            run(*fill[j * 4 // NJ])
    for j in range(NJ):
        recv(send_part(j))
        run(o_own(j, j == 0))
        out_store(j).start()
    for j in range(NJ):
        out_store(j).wait()
    if not NOCOMM:
        for t in all4:
            send_x(t).wait_send()
            send_wq(t).wait_send()
        for j in range(NJ):
            send_wo(j).wait_send()
            send_part(j).wait_send()


def pallas_dist_sparse_attn_strided_qseq_b1_sq1024_skv1024_hq8_dh128_kernel(x, Wq, K_ext, V_ext, Wo):
    hbm = pl.BlockSpec(memory_space=pltpu.HBM)
    dma = pltpu.SemaphoreType.DMA
    flags = {f: True for f in E("FLAGS", "").split(",") if f}
    return pl.pallas_call(
        _body,
        out_shape=jax.ShapeDtypeStruct((1, 1024, 1024), F32),
        in_specs=[hbm] * 5,
        out_specs=hbm,
        scratch_shapes=[
            pltpu.VMEM((1024, 1024), F32), pltpu.VMEM((1024, 1024), F32), pltpu.VMEM((1024, 1024), F32),
            pltpu.VMEM((2, 4, 8, 4, 64, 128), F32), pltpu.VMEM((2, 4, 8, 4, 64, 128), F32),
            pltpu.VMEM((2, 4, 256, 1024), BF16), pltpu.VMEM((2, 4, 1024, 256), BF16),
            pltpu.VMEM((2, NJ, 1024, CW), BF16),
            pltpu.VMEM((2, 4, 8, 256, 128), BF16), pltpu.VMEM((2, 4, 8, 256, 128), BF16),
            pltpu.VMEM((2, 1024, 2048), BF16), pltpu.VMEM((2, 1024, 2048), BF16),
            pltpu.VMEM((2, 1024, 1024), F32),
            pltpu.VMEM((NJ, 1024, CW), BF16), pltpu.VMEM((NJ, 1024, CW), BF16),
            dma((NKC,)), dma((NKC,)), dma, dma((2, 2, 4)), dma((NJ,)),
            dma((4,)), dma((4,)), dma((4,)), dma((4,)), dma((NJ,)), dma((NJ,)), dma((NJ,)), dma((NJ,)),
        ],
        compiler_params=pltpu.CompilerParams(
            collective_id=None if NOCOMM else 0, vmem_limit_bytes=110 << 20, flags=flags or None),
    )(x, Wq, K_ext.reshape(4, 4, 64, 32, 128), V_ext.reshape(4, 4, 64, 32, 128), Wo)
```

```python
import contextlib
import os
import jax
import jax.numpy as jnp
from jax import lax
from jax.experimental import pallas as pl
from jax.experimental.pallas import tpu as pltpu

E = os.environ.get
NOCOMM = int(E("NOCOMM", 0))
LOOK = int(E("LOOK", 4))
BAR = int(E("BAR", 1))
AHEAD = int(E("AHEAD", 2))
TAIL0 = int(E("TAIL0", 2))
PRX = int(E("PRX", 0))
LATE = int(E("LATE", 1))
PRI = int(E("PRI", 0))
L1 = int(E("L1", 4))
L2 = int(E("L2", 8))
L3 = int(E("L3", 11))
SPLIT = int(E("SPLIT", 4))
HOLD = int(E("HOLD", 8))
A0 = int(E("A0", 0))
A1 = int(E("A1", 7))
A2 = int(E("A2", 15))
KEEP = int(E("KEEP", 7))
STRIP = int(E("STRIP", 32))
F1 = int(E("F1", 8))
F2 = int(E("F2", 11))
F3 = int(E("F3", 1))
F4 = int(E("F4", 6))
SCOPES = int(E("SCOPES", 0))
KC = 128
NKC = 1024 // KC
F32, BF16 = jnp.float32, jnp.bfloat16
QSCALE = 0.08838834764831843 * 1.4426950408889634


class _Job:
    def __init__(self, fn, args=(), needs=(), gives=(), cost=1.0, quiet=False):
        self.fn, self.args, self.needs, self.gives, self.cost = fn, args, set(needs), set(gives), cost
        self.quiet = quiet


def _interleave(done, lists):
    lists = [list(js) for js in lists if js]
    total = [sum(j.cost for j in js) for js in lists]
    spent = [0.0] * len(lists)
    order = []
    while any(lists):
        ready = [n for n, js in enumerate(lists) if js and js[0].needs <= done]
        assert ready, [js[0].needs - done for js in lists if js]
        n = min(ready, key=lambda n: (spent[n] + lists[n][0].cost / 2) / total[n])
        job = lists[n].pop(0)
        spent[n] += job.cost
        done |= job.gives
        order.append(job)
    return order


def _lhs_sums(a11, a12, a21, a22):
    return a11 + a22, a21 + a22, a11 + a12, a21 - a11, a12 - a22


def _rhs_sums(b11, b12, b21, b22):
    return b11 + b22, b12 - b22, b21 - b11, b11 + b12, b21 + b22


def _mm(a, b):
    return jnp.dot(a, b, preferred_element_type=F32)


class _Packed:
    def __init__(self, refs):
        self.refs = refs

    def _pick(self, idx):
        ref = self.refs
        while isinstance(ref, (list, tuple)):
            ref, idx = ref[idx[0]], idx[1:]
        return ref, idx + (slice(None),) * (len(ref.shape) - len(idx))

    def __getitem__(self, idx):
        ref, idx = self._pick(idx)
        r = idx[-2]
        idx = idx[:-2] + (slice(None) if r.stop is None else slice(r.start // 2, r.stop // 2), idx[-1])
        return pltpu.bitcast(ref.bitcast(jnp.uint32)[idx], BF16)

    def __setitem__(self, idx, value):
        ref, idx = self._pick(idx)
        ref[idx] = value.astype(BF16)


def _buffers(lead, shape, dtype):
    if not lead:
        return pltpu.VMEM(shape, dtype)
    return [_buffers(lead[1:], shape, dtype) for _ in range(lead[0])]


def _wide(buf, idx, blocks, rows=slice(None)):
    return jnp.concatenate([buf[(*idx, k, rows)] for k in blocks], axis=1)


def _strassen(product, put, needs, gives=()):
    m = {}

    def step(n):
        y = product(n)
        if n == 2:
            m["22"] = y
        elif n == 4:
            put(2, m["22"] + y)
            m["11"] = y
        elif n == 3:
            m["12"] = y
            m["22"] = y - m["22"]
        elif n == 5:
            put(1, m.pop("12") + y)
            m["11"] = m["11"] - y
        elif n == 1:
            m["11"], m["22"] = m["11"] + y, m["22"] + y
        elif n == 7:
            put(0, m.pop("11") + y)
        else:
            put(3, m.pop("22") + y)

    return [_Job(step, (n,), needs if n == 2 else (), gives if n == 6 else (), quiet=n < 4)
            for n in (2, 4, 3, 5, 1, 7, 6)]


def _body(x_hbm, wq_hbm, k_hbm, v_hbm, wo_hbm, out,
          xf, wqf, wof, kvf, xb, xs, wqb, wqs, wob, wos, qb, cs, sbuf, rbuf,
          x_sem, wq_sem, wo_sem, kv_sem, tx_x, rx_x, tx_q, rx_q, tx_o, rx_o, tx_p, rx_p):
    me = lax.axis_index("i")
    row_peer = me ^ 1
    head_peer = 3 - me
    mesh_id = pl.DeviceIdType.MESH
    lo, hi = slice(0, 512), slice(512, 1024)
    all4 = range(4)
    done = {("x", 0, m) for m in all4} | {("wq", 0, j) for j in all4}
    xb, xs, wqb, wqs, wob, wos, qb, cs, sbuf, rbuf = map(
        _Packed, (xb, xs, wqb, wqs, wob, wos, qb, cs, sbuf, rbuf))

    if not NOCOMM:
        barrier = pltpu.get_barrier_semaphore()
        for peer in (row_peer, head_peer):
            pl.semaphore_signal(barrier, inc=1, device_id=(peer,), device_id_type=mesh_id)

    halves = (pl.ds(0, 512), pl.ds(512, 512), slice(None))

    def x_load(m, part=2):
        c = halves[part]
        return pltpu.make_async_copy(x_hbm.at[:, m, :, c], xf.at[m, :, :, c], x_sem.at[m + (part > 0)])

    def wq_load(j, part=2):
        r = halves[part]
        return pltpu.make_async_copy(wq_hbm.at[r, pl.ds(j * 256, 256)], wqf.at[j, r], wq_sem.at[j + (part > 0)])

    def wo_load(j):
        return pltpu.make_async_copy(wo_hbm.at[:, pl.ds(j * 256, 256)], wof.at[j], wo_sem.at[j])

    def kv_start(g, m):
        head0 = (me if g == 0 else head_peer) * 8
        for t, src in enumerate((k_hbm, v_hbm)):
            for h in range(8):
                pltpu.make_async_copy(src.at[:, m, :, head0 + h, :], kvf.at[g, m, t, h], kv_sem.at[g, m]).start()

    def kv_wait(g, m):
        pltpu.make_async_copy(kvf.at[g, m], kvf.at[g, m], kv_sem.at[g, m]).wait()
        done.add(("kv", g, m))

    def remote(src, dst, tx, rx, peer):
        return pltpu.make_async_remote_copy(src, dst, tx, rx, device_id=(peer,), device_id_type=mesh_id)

    def send_x(m, c=slice(None)):
        return remote(xb.refs[0][m].at[c], xb.refs[1][m].at[c], tx_x.at[m], rx_x.at[m], row_peer)

    def send_wq(j, r=slice(None)):
        return remote(wqb.refs[0][j].at[r], wqb.refs[1][j].at[r], tx_q.at[j], rx_q.at[j], head_peer)

    def send_wo(j):
        return remote(wob.refs[0][j], wob.refs[1][j], tx_o.at[j], rx_o.at[j], head_peer)

    def send_part(j, m):
        rx = rx_p.at[j + (m if j == 3 else 0)]
        return remote(sbuf.refs.at[j, m], rbuf.refs[j].at[m], tx_p, rx, row_peer)

    def send_chunk(j):
        return remote(sbuf.refs.at[j], rbuf.refs[j], tx_p, rx_p.at[j], row_peer)

    def start(mk, *a):
        assert not any(job.fn is cast_wo for job in carried)
        if not NOCOMM:
            mk(*a).start()

    def recv(mk, *a):
        if not NOCOMM:
            with jax.named_scope("z_" + mk.__name__[5:] + "".join(map(str, a))) if SCOPES else contextlib.nullcontext():
                mk(*a).wait_recv()

    def strips(fn, items, needs, gives):
        rows = [slice(u * STRIP, (u + 1) * STRIP) for u in range(128 // STRIP)]
        return [_Job(fn, (*it, r), needs(*it), gives(*it) if r is rows[-1] else ()) for it in items for r in rows]

    def sum_x(s, m, k, r):
        if s == 0:
            a, t = divmod(r.start, 64)
            quads = [xf[m, 2 * e + a, t:t + STRIP, kk * 128:(kk + 1) * 128] for e in range(2) for kk in (k, k + 4)]
        else:
            quads = [xb[s, m, kk, e * 128 + r.start:e * 128 + r.stop].astype(F32) for e in range(2) for kk in (k, k + 4)]
        for i, v in enumerate(_lhs_sums(*quads)):
            xs[s, m, k, i, r] = v

    def x_sums(s, m):
        return strips(sum_x, [(s, m, k) for k in all4], lambda s, m, k: [("x", s, m)], lambda *it: [("xs", *it)])

    def sum_wq(g, j, k, r):
        if g == 0:
            quads = [wqf[j, kk * 128 + r.start:kk * 128 + r.stop, c * 128:(c + 1) * 128] * QSCALE
                     for kk in (k, k + 4) for c in range(2)]
        else:
            quads = [wqb[g, j, kk, c, r].astype(F32) for kk in (k, k + 4) for c in range(2)]
        for i, v in enumerate(_rhs_sums(*quads)):
            wqs[g, j, k, i, r] = v

    def wq_sums(g, j):
        return strips(sum_wq, [(g, j, k) for k in all4], lambda g, j, k: [("wq", g, j)], lambda *it: [("wqs", *it)])

    def wo_quads(j, p, r):
        return [wof[j, (2 * p + e) * 128 + r.start:(2 * p + e) * 128 + r.stop, c * 128:(c + 1) * 128]
                for e in range(2) for c in range(2)]

    def cast_wo(j, p, r):
        for n, v in enumerate(wo_quads(j, p, r)):
            wob[0, j, n % 2, n // 2, p * 128 + r.start:p * 128 + r.stop] = v

    def sum_wo(g, j, p, r):
        rows = slice(p * 128 + r.start, p * 128 + r.stop)
        quads = wo_quads(j, p, r) if g == 0 else [wob[g, j, c, e, rows].astype(F32) for e in range(2) for c in range(2)]
        for i, v in enumerate(_rhs_sums(*quads)):
            wos[g, j, i, rows] = v

    def wo_cast(j):
        return strips(cast_wo, [(j, p) for p in all4], lambda *it: (), lambda *it: [("wo", *it)])

    def wo_sums(j, g=0):
        return strips(sum_wo, [(g, j, p) for p in all4], lambda *it: (), lambda *it: [("wos", *it)])

    def q_block(s, m, g, j):
        def product(n):
            if n in (3, 4):
                left = [xb[s, m, k + 4 * (n - 3), (n - 3) * 128:(n - 2) * 128] for k in all4]
            else:
                left = [xs[s, m, k, {1: 0, 2: 1, 5: 2, 6: 3, 7: 4}[n]] for k in all4]
            if n in (2, 5):
                right = [wqb[g, j, k + 4 * (n // 5), n // 5] for k in all4]
            else:
                right = [wqs[g, j, k, {1: 0, 3: 1, 4: 2, 6: 3, 7: 4}[n]] for k in all4]
            return _mm(jnp.concatenate(left, axis=1), jnp.concatenate(right, axis=0))

        def put(q, y):
            qb[s, m, g, j, q % 2, q // 2 * 128:(q // 2 + 1) * 128] = y

        needs = [("xs", s, m, k) for k in all4] + [("wqs", g, j, k) for k in all4]
        return _strassen(product, put, needs, [("q", s, m, g, j)])

    def q_proj(items):
        return [job for it in items for job in q_block(*it)]

    def attn(pairs):
        items = [(s, m, g, j, r, e) for s, m, g, j in pairs for r, e in ((0, 0), (1, 1), (0, 1), (1, 0))]
        live = {}

        def scores(n):
            s, m, g, j, r, e = items[n]
            q = qb[s, m, g, j, e, r * 128:(r + 1) * 128, :]
            k = kvf[g, m, 0, 2 * j + e].reshape(256, 128).astype(BF16)
            sc = lax.dot_general(q, k, (((1,), (1,)), ((), ())), preferred_element_type=F32)
            p = jnp.exp2(sc - jnp.max(sc, axis=1, keepdims=True))
            live[n] = (p.astype(BF16), jnp.sum(p, axis=1, keepdims=True))

        def context(n):
            s, m, g, j, r, e = items[n]
            p, l = live.pop(n)
            v = kvf[g, m, 1, 2 * j + e].reshape(256, 128).astype(BF16)
            o = _mm(p, v) * pl.reciprocal(l, approx=True)

            def put(i, value):
                cs[s, g, i, j, m * 128:(m + 1) * 128, :] = value

            if (r, e) == (0, 0):
                live["11"] = o
                put(5, o)
            elif (r, e) == (1, 1):
                live["22"] = o
                put(6, o)
                put(0, live["11"] + o)
            elif (r, e) == (0, 1):
                put(2, live["11"] + o)
                put(4, o - live["22"])
            else:
                put(3, o - live.pop("11"))
                put(1, o + live.pop("22"))

        out_jobs = []
        for n in range(len(items) + LOOK):
            if n < len(items):
                s, m, g, j = items[n][:4]
                out_jobs.append(_Job(scores, (n,), [("q", s, m, g, j), ("kv", g, m)]))
            if n >= LOOK:
                last = (n - LOOK) % 4 == 3
                out_jobs.append(_Job(context, (n - LOOK,), (), [("c",) + items[n - LOOK][:4]] * last))
        return out_jobs

    def o_prod(s, j, m, n):
        i = (0, 1, 5, 6, 2, 3, 4)[n - 1]
        left = jnp.concatenate([cs[s, g, i, p, m * 128:(m + 1) * 128] for g in range(2) for p in all4], axis=1)
        if n in (2, 5):
            right = [wob[g, j, n // 5, n // 5] for g in range(2)]
        else:
            right = [wos[g, j, {1: 0, 3: 1, 4: 2, 6: 3, 7: 4}[n]] for g in range(2)]
        return _mm(left, jnp.concatenate(right, axis=0))

    def o_block(s, j, m, put):
        needs = [("c", s, m, g, p) for g in range(2) for p in all4]
        needs += [("wo", j, p) for p in all4] + [("wos", g, j, p) for g in range(2) for p in all4]
        return _strassen(lambda n: o_prod(s, j, m, n), put, needs)

    def finish(j, m, q, y):
        y = (y + rbuf[j, m, q].astype(F32)).astype(out.dtype)
        r, c = divmod(q, 2)
        for u in range(2):
            r0 = (4 * (2 * r + u) + m) * 64
            out[0, r0:r0 + 64, j * 256 + c * 128:j * 256 + (c + 1) * 128] = y[u * 64:(u + 1) * 64]

    def o_own(j, m):
        return o_block(0, j, m, lambda q, y: finish(j, m, q, y))

    def o_peer(j, m):
        def put(q, y):
            sbuf[j, m, q] = y
        return o_block(1, j, m, put)

    carried = []

    def run(*lists, flush=False):
        order = carried + _interleave(done, lists)
        quiet = [n + 1 for n, job in enumerate(order) if job.quiet]
        stop = quiet[-1] if quiet and not flush else len(order)
        for job in order[:stop]:
            job.fn(*job.args)
        carried[:] = order[stop:]

    def grid(s, ms, g, js):
        return [(s, m, g, j) for m in ms for j in js]

    def cast_x(m, kc):
        xb[0, m, kc] = xf[m, :, :, kc * 128:(kc + 1) * 128].reshape(256, 128)

    def cast_wq(j, kc):
        for e in range(2):
            wqb[0, j, kc, e] = wqf[j, kc * 128:(kc + 1) * 128, e * 128:(e + 1) * 128] * QSCALE

    for part in range(2):
        x_load(0, part).start()
        wq_load(0, part).start()
    for part in range(2):
        x_load(0, part).wait()
        wq_load(0, part).wait()
        (x_load, wq_load)[part](1).start()
        run([_Job(fn, (0, 4 * part + k)) for k in all4 for fn in (cast_x, cast_wq)], flush=True)
        if part == 0 and not NOCOMM:
            pl.semaphore_wait(barrier, 2)
        start(send_x, 0, pl.ds(4 * part, 4))
        start(send_wq, 0, pl.ds(4 * part, 4))
    run(x_sums(0, 0) + wq_sums(0, 0) + q_proj([(0, 0, 0, 0)]))
    work = []
    for t in (1, 2, 3):
        x_load(t).wait()
        if t < 3:
            x_load(t + 1).start()
        else:
            kv_start(0, 0)
        run(work, [_Job(cast_x, (t, kc)) for kc in range(8)] + x_sums(0, t), flush=True)
        start(send_x, t)
        blocks = q_proj(grid(0, [t], 0, range(t)))
        keep = max(len(blocks) - KEEP, 0)
        run(blocks[:keep])
        wq_load(t).wait()
        if t < 3:
            wq_load(t + 1).start()
        else:
            kv_start(0, 1)
        run(blocks[keep:], [_Job(cast_wq, (t, kc)) for kc in range(8)] + wq_sums(0, t), flush=True)
        start(send_wq, t)
        blocks = q_proj(grid(0, range(t + 1), 0, [t]))
        keep = 14 if t == 3 else KEEP
        run(blocks[:-keep])
        work = blocks[-keep:]

    def got(t):
        recv(send_x, t)
        recv(send_wq, t)
        done.update([("x", 1, t), ("wq", 1, t)])

    def early(js, share):
        return js + [_Job(lambda: None, cost=len(js) * (1 / share - 1))]

    new1 = [(1, 1, 1, 0), (1, 0, 1, 1), (1, 1, 1, 1)]
    new2 = grid(1, [0, 1], 1, [2]) + grid(1, [2], 1, [0, 1, 2])
    new3 = grid(1, [0, 1, 2], 1, [3]) + grid(1, [3], 1, all4) + grid(1, [3], 0, all4)
    own = [(0, m, 1, j) for j in all4 for m in all4]

    run(work[:-7])
    kv_wait(0, 0)
    run(work[-7:], attn(grid(0, [0], 0, all4)))
    kv_start(1, 0)
    got(0)
    run(q_proj(grid(1, [0], 0, all4)), x_sums(1, 0) + wq_sums(1, 0))
    kv_start(1, 1)
    kv_wait(0, 1)
    run(q_proj([(1, 0, 1, 0)] + own[:4]), attn(grid(1, [0], 0, all4) + grid(0, [1], 0, all4)))
    wo_load(0).start()
    kv_start(0, 2)
    got(1)
    run(q_proj(grid(1, [1], 0, all4) + new1 + own[4:5]), attn(grid(1, [1], 0, all4)),
        early(x_sums(1, 1) + wq_sums(1, 1), 0.4))
    wo_load(1).start()
    kv_start(1, 2)
    kv_wait(1, 0)
    kv_wait(1, 1)
    kv_wait(0, 2)
    run(q_proj(own[5:F1]), attn([(1, 0, 1, 0)] + new1 + grid(0, [2], 0, [0, 1])))
    kv_start(0, 3)
    kv_start(1, 3)
    wo_load(2).start()
    wo_load(3).start()
    wo_load(0).wait()
    got(2)
    run(q_proj(grid(1, [2], 0, all4) + new2 + own[F1:F1 + 1]), attn(grid(0, [2], 0, [2, 3]) + grid(1, [2], 0, all4) + new2[:2]),
        early(x_sums(1, 2) + wq_sums(1, 2) + wo_cast(0), 0.8))
    start(send_wo, 0)
    kv_wait(1, 2)
    wo_load(1).wait()
    run(q_proj(own[F1 + 1:F2]), attn(new2[2:] + own[:2]), early(wo_cast(1), 0.7))
    start(send_wo, 1)
    kv_wait(0, 3)
    kv_wait(1, 3)
    got(3)
    run(q_proj(own[F2:F2 + 1] + new3), attn(grid(0, [3], 0, range(A0)) + new3), early(wq_sums(1, 3) + x_sums(1, 3), 0.4) + wo_sums(0))
    for j in (2, 3):
        wo_load(j).wait()

    mine = [o_own(j, m) for j in all4 for m in all4]

    def peer_rows(j):
        jobs = []
        for m in all4:
            block = o_peer(j, m)
            jobs += block[:1] + [_Job(start, (send_part, j, m - 1), cost=0)] * (m > 0) + block[1:]
        return jobs

    def send_last(j, jobs):
        return jobs[:1] + [_Job(start, (send_part, j, 3), cost=0)] + jobs[1:]

    def got_wo(j):
        recv(send_wo, j)
        return wo_sums(j, 1)

    run(q_proj(own[12:13]) + peer_rows(0), early(got_wo(0), 0.3) + early(wo_cast(2), 0.5))
    start(send_wo, 2)
    run(send_last(0, q_proj(own[13:15])), attn(grid(0, [3], 0, range(A0, 4)) + own[2:A1]), early(wo_cast(3) + wo_sums(1), 0.75))
    start(send_wo, 3)
    run(q_proj(own[15:]) + peer_rows(1), early(got_wo(1), 0.25) + wo_sums(2))
    run(send_last(1, attn(own[A1:])))
    recv(send_chunk, 0)
    run(mine[0], wo_sums(3))
    run(mine[1] + peer_rows(2), got_wo(2))
    run(send_last(2, mine[2] + mine[3]))
    recv(send_chunk, 1)
    run(sum(mine[4:F4], []))
    run(mine[F4] + peer_rows(3), got_wo(3))
    for t in all4:
        send_x(t).wait_send()
        send_wq(t).wait_send()
        send_wo(t).wait_send()
    run(send_last(3, sum(mine[F4 + 1:8], [])))
    recv(send_chunk, 2)
    run(sum(mine[8:12], []))
    for m in range(3):
        recv(send_part, 3, m)
        run(mine[12 + m])
    last = []
    run(o_block(0, 3, 3, lambda q, y: last.append((q, y))), flush=True)
    recv(send_part, 3, 3)
    for q, y in last:
        finish(3, 3, q, y)
    remote(sbuf.refs, sbuf.refs, tx_p, rx_p.at[0], row_peer).wait_send()


def pallas_dist_sparse_attn_strided_qseq_b1_sq1024_skv1024_hq8_dh128_kernel(x, Wq, K_ext, V_ext, Wo):
    hbm = pl.BlockSpec(memory_space=pltpu.HBM)
    dma = pltpu.SemaphoreType.DMA
    flags = {f: True for f in E("FLAGS", "").split(",") if f}
    return pl.pallas_call(
        _body,
        out_shape=jax.ShapeDtypeStruct((1, 1024, 1024), BF16),
        in_specs=[hbm] * 5,
        out_specs=pl.BlockSpec(memory_space=pltpu.VMEM),
        scratch_shapes=[
            pltpu.VMEM((4, 4, 64, 1024), F32), pltpu.VMEM((4, 1024, 256), F32), pltpu.VMEM((4, 1024, 256), F32),
            pltpu.VMEM((2, 4, 2, 8, 4, 64, 128), F32),
            _buffers((2, 4), (8, 256, 128), BF16), _buffers((2, 4), (4, 5, 128, 128), BF16),
            _buffers((2, 4), (8, 2, 128, 128), BF16), _buffers((2, 4), (4, 5, 128, 128), BF16),
            _buffers((2, 4), (2, 2, 512, 128), BF16), _buffers((2, 4), (5, 512, 128), BF16),
            _buffers((2, 4, 2, 4), (2, 256, 128), BF16), _buffers((2, 2), (7, 4, 512, 128), BF16),
            pltpu.VMEM((4, 4, 4, 128, 128), BF16), _buffers((4,), (4, 4, 128, 128), BF16),
            dma((5,)), dma((5,)), dma((4,)), dma((2, 4)),
            dma((4,)), dma((4,)), dma((4,)), dma((4,)), dma((4,)), dma((4,)), dma, dma((7,)),
        ],
        compiler_params=pltpu.CompilerParams(
            collective_id=None if NOCOMM else 0, vmem_limit_bytes=110 << 20, flags=flags or None),
    )(x.reshape(4, 4, 64, 1024), Wq, K_ext.reshape(4, 4, 64, 32, 128), V_ext.reshape(4, 4, 64, 32, 128), Wo)
```

```python
import jax
import jax.numpy as jnp
from jax import lax
from jax.experimental import pallas as pl
from jax.experimental.pallas import tpu as pltpu

F32, BF16 = jnp.float32, jnp.bfloat16
QSCALE = 0.08838834764831843 * 1.4426950408889634
LOOK = 4
STRIP = 64
KEEP = 7


class _Job:
    def __init__(self, fn, args=(), needs=(), gives=(), cost=1.0, quiet=False):
        self.fn, self.args, self.needs, self.gives, self.cost = fn, args, set(needs), set(gives), cost
        self.quiet = quiet


def _interleave(done, lists):
    lists = [list(js) for js in lists if js]
    total = [sum(j.cost for j in js) for js in lists]
    spent = [0.0] * len(lists)
    order = []
    while any(lists):
        ready = [n for n, js in enumerate(lists) if js and js[0].needs <= done]
        assert ready, [js[0].needs - done for js in lists if js]
        n = min(ready, key=lambda n: (spent[n] + lists[n][0].cost / 2) / total[n])
        job = lists[n].pop(0)
        spent[n] += job.cost
        done |= job.gives
        order.append(job)
    return order


def _lhs_sums(a11, a12, a21, a22):
    return a11 + a22, a21 + a22, a11 + a12, a21 - a11, a12 - a22


def _rhs_sums(b11, b12, b21, b22):
    return b11 + b22, b12 - b22, b21 - b11, b11 + b12, b21 + b22


def _mm(a, b):
    return jnp.dot(a, b, preferred_element_type=F32)


class _Packed:
    def __init__(self, refs):
        self.refs = refs

    def _pick(self, idx):
        ref = self.refs
        while isinstance(ref, (list, tuple)):
            ref, idx = ref[idx[0]], idx[1:]
        return ref, idx + (slice(None),) * (len(ref.shape) - len(idx))

    def __getitem__(self, idx):
        ref, idx = self._pick(idx)
        r = idx[-2]
        idx = idx[:-2] + (slice(None) if r.stop is None else slice(r.start // 2, r.stop // 2), idx[-1])
        return pltpu.bitcast(ref.bitcast(jnp.uint32)[idx], BF16)

    def __setitem__(self, idx, value):
        ref, idx = self._pick(idx)
        ref[idx] = value.astype(BF16)


def _buffers(lead, shape, dtype):
    if not lead:
        return pltpu.VMEM(shape, dtype)
    return [_buffers(lead[1:], shape, dtype) for _ in range(lead[0])]


def _wide(buf, idx, blocks, rows=slice(None)):
    return jnp.concatenate([buf[(*idx, k, rows)] for k in blocks], axis=1)


def _side_by_side(*stacks):
    tall = [stack.reshape(512, 128) for stack in stacks]
    return lax.concatenate([lax.slice_in_dim(t, k * 128, (k + 1) * 128) for t in tall for k in range(4)], 1)


def _strassen(product, put, needs, gives=()):
    m = {}

    def step(n):
        y = product(n)
        if n == 2:
            m["22"] = y
        elif n == 4:
            put(2, m["22"] + y)
            m["11"] = y
        elif n == 3:
            m["12"] = y
            m["22"] = y - m["22"]
        elif n == 5:
            put(1, m.pop("12") + y)
            m["11"] = m["11"] - y
        elif n == 1:
            m["11"], m["22"] = m["11"] + y, m["22"] + y
        elif n == 7:
            put(0, m.pop("11") + y)
        else:
            put(3, m.pop("22") + y)

    return [_Job(step, (n,), needs if n == 2 else (), gives if n == 6 else (), quiet=n < 4)
            for n in (2, 4, 3, 5, 1, 7, 6)]


def _body(x_hbm, wq_hbm, k_hbm, v_hbm, wo_hbm, out,
          xf, wqf, wof, kvf, xb, xs, wqb, wqs, wob, wos, qb, cs, sbuf, rbuf,
          x_sem, wq_sem, wo_sem, kv_sem, tx_x, rx_x, tx_q, rx_q, tx_o, rx_o, tx_p, rx_p):
    me = lax.axis_index("i")
    row_peer = me ^ 1
    head_peer = 3 - me
    mesh_id = pl.DeviceIdType.MESH
    lo, hi = slice(0, 512), slice(512, 1024)
    all4 = range(4)
    done = {("x", 0, m) for m in all4} | {("wq", 0, j) for j in all4}
    xb, xs, wqb, wqs, wob, wos, qb, cs, sbuf, rbuf = map(
        _Packed, (xb, xs, wqb, wqs, wob, wos, qb, cs, sbuf, rbuf))

    barrier = pltpu.get_barrier_semaphore()
    for peer in (row_peer, head_peer):
        pl.semaphore_signal(barrier, inc=1, device_id=(peer,), device_id_type=mesh_id)

    halves = (pl.ds(0, 512), pl.ds(512, 512), slice(None))

    def x_load(m, part=2):
        c = halves[part]
        return pltpu.make_async_copy(x_hbm.at[:, m, :, c], xf.at[m, :, :, c], x_sem.at[m + (part > 0)])

    def wq_load(j, part=2):
        r = halves[part]
        return pltpu.make_async_copy(wq_hbm.at[r, pl.ds(j * 256, 256)], wqf.at[j, r], wq_sem.at[j + (part > 0)])

    def wo_load(j):
        return pltpu.make_async_copy(wo_hbm.at[:, pl.ds(j * 256, 256)], wof.at[j], wo_sem.at[j])

    def kv_start(g, m):
        head0 = (me if g == 0 else head_peer) * 8
        for h in range(8):
            sem = kv_sem.at[0, 4] if (g, m) == (0, 0) and h >= 4 else kv_sem.at[g, m]
            for t, src in enumerate((k_hbm, v_hbm)):
                pltpu.make_async_copy(src.at[:, m, :, head0 + h, :], kvf.at[g, m, h, t], sem).start()

    def kv_wait(g, m, half=None):
        heads = slice(None) if half is None else pl.ds(4 * half, 4)
        sem = kv_sem.at[0, 4] if half else kv_sem.at[g, m]
        pltpu.make_async_copy(kvf.at[g, m, heads], kvf.at[g, m, heads], sem).wait()
        done.update(("kv", g, m, j) for j in all4 if half is None or j // 2 == half)

    def remote(src, dst, tx, rx, peer):
        return pltpu.make_async_remote_copy(src, dst, tx, rx, device_id=(peer,), device_id_type=mesh_id)

    def send_x(m, c=slice(None)):
        return remote(xb.refs[0][m].at[c], xb.refs[1][m].at[c], tx_x.at[m], rx_x.at[m], row_peer)

    def send_wq(j, r=slice(None)):
        return remote(wqb.refs[0][j].at[r], wqb.refs[1][j].at[r], tx_q.at[j], rx_q.at[j], head_peer)

    def send_wo(j):
        return remote(wob.refs[0][j], wob.refs[1][j], tx_o.at[j], rx_o.at[j], head_peer)

    def send_part(j, m):
        rx = rx_p.at[j + (m if j == 3 else 0)]
        return remote(sbuf.refs.at[j, m], rbuf.refs[j].at[m], tx_p, rx, row_peer)

    def send_chunk(j):
        return remote(sbuf.refs.at[j], rbuf.refs[j], tx_p, rx_p.at[j], row_peer)

    def start(make, *args):
        assert not any(job.fn is cast_wo for job in carried)
        make(*args).start()

    def recv(make, *args):
        make(*args).wait_recv()

    def strips(fn, items, needs, gives):
        rows = [slice(u * STRIP, (u + 1) * STRIP) for u in range(128 // STRIP)]
        return [_Job(fn, (*it, r), needs(*it), gives(*it) if r is rows[-1] else ()) for it in items for r in rows]

    def sum_x(s, m, k, r):
        if s == 0:
            a, t = divmod(r.start, 64)
            quads = [xf[m, 2 * e + a, t:t + STRIP, kk * 128:(kk + 1) * 128] for e in range(2) for kk in (k, k + 4)]
        else:
            quads = [xb[s, m, kk, e * 128 + r.start:e * 128 + r.stop].astype(F32) for e in range(2) for kk in (k, k + 4)]
        for i, v in enumerate(_lhs_sums(*quads)):
            xs[s, m, k, i, r] = v

    def x_sums(s, m):
        return strips(sum_x, [(s, m, k) for k in all4], lambda s, m, k: [("x", s, m)], lambda *it: [("xs", *it)])

    def sum_wq(g, j, k, r):
        if g == 0:
            quads = [wqf[j, kk * 128 + r.start:kk * 128 + r.stop, c * 128:(c + 1) * 128] * QSCALE
                     for kk in (k, k + 4) for c in range(2)]
        else:
            quads = [wqb[g, j, kk, c, r].astype(F32) for kk in (k, k + 4) for c in range(2)]
        for i, v in enumerate(_rhs_sums(*quads)):
            wqs[g, j, k, i, r] = v

    def wq_sums(g, j):
        return strips(sum_wq, [(g, j, k) for k in all4], lambda g, j, k: [("wq", g, j)], lambda *it: [("wqs", *it)])

    def wo_quads(j, p, r):
        return [wof[j, (2 * p + e) * 128 + r.start:(2 * p + e) * 128 + r.stop, c * 128:(c + 1) * 128]
                for e in range(2) for c in range(2)]

    def cast_wo(j, p, r):
        for n, v in enumerate(wo_quads(j, p, r)):
            wob[0, j, n % 2, n // 2, p * 128 + r.start:p * 128 + r.stop] = v

    def sum_wo(g, j, p, r):
        rows = slice(p * 128 + r.start, p * 128 + r.stop)
        quads = wo_quads(j, p, r) if g == 0 else [wob[g, j, c, e, rows].astype(F32) for e in range(2) for c in range(2)]
        for i, v in enumerate(_rhs_sums(*quads)):
            wos[g, j, i, rows] = v

    def wo_cast(j):
        return strips(cast_wo, [(j, p) for p in all4], lambda *it: (), lambda *it: [("wo", *it)])

    def wo_sums(j, g=0):
        return strips(sum_wo, [(g, j, p) for p in all4], lambda *it: (), lambda *it: [("wos", *it)])

    def q_block(s, m, g, j):
        def product(n):
            if n in (3, 4):
                left = xb[s, m, 4 * (n - 3):4 * (n - 2), (n - 3) * 128:(n - 2) * 128]
            else:
                left = xs[s, m, :, {1: 0, 2: 1, 5: 2, 6: 3, 7: 4}[n]]
            if n in (2, 5):
                right = wqb[g, j, 4 * (n // 5):4 * (n // 5) + 4, n // 5]
            else:
                right = wqs[g, j, :, {1: 0, 3: 1, 4: 2, 6: 3, 7: 4}[n]]
            return _mm(_side_by_side(left), right.reshape(512, 128))

        def put(q, y):
            qb[s, m, g, j, q % 2, q // 2 * 128:(q // 2 + 1) * 128] = y

        needs = [("xs", s, m, k) for k in all4] + [("wqs", g, j, k) for k in all4]
        return _strassen(product, put, needs, [("q", s, m, g, j)])

    def q_proj(items):
        return [job for it in items for job in q_block(*it)]

    def attn(pairs):
        items = [(s, m, g, j, r, e) for s, m, g, j in pairs for r, e in ((0, 0), (1, 1), (0, 1), (1, 0))]
        live = {}

        def scores(n):
            s, m, g, j, r, e = items[n]
            q = qb[s, m, g, j, e, r * 128:(r + 1) * 128, :]
            k = kvf[g, m, 2 * j + e, 0].reshape(256, 128).astype(BF16)
            sc = lax.dot_general(q, k, (((1,), (1,)), ((), ())), preferred_element_type=F32)
            p = jnp.exp2(sc - jnp.max(sc, axis=1, keepdims=True))
            live[n] = (p.astype(BF16), jnp.sum(p, axis=1, keepdims=True))

        def context(n):
            s, m, g, j, r, e = items[n]
            p, l = live.pop(n)
            v = kvf[g, m, 2 * j + e, 1].reshape(256, 128).astype(BF16)
            o = _mm(p, v) * pl.reciprocal(l, approx=True)

            def put(i, value):
                cs[s, g, i, j, m * 128:(m + 1) * 128, :] = value

            if (r, e) == (0, 0):
                live["11"] = o
                put(5, o)
            elif (r, e) == (1, 1):
                live["22"] = o
                put(6, o)
                put(0, live["11"] + o)
            elif (r, e) == (0, 1):
                put(2, live["11"] + o)
                put(4, o - live["22"])
            else:
                put(3, o - live.pop("11"))
                put(1, o + live.pop("22"))

        out_jobs = []
        for n in range(len(items) + LOOK):
            if n < len(items):
                s, m, g, j = items[n][:4]
                out_jobs.append(_Job(scores, (n,), [("q", s, m, g, j), ("kv", g, m, j)]))
            if n >= LOOK:
                last = (n - LOOK) % 4 == 3
                out_jobs.append(_Job(context, (n - LOOK,), (), [("c",) + items[n - LOOK][:4]] * last))
        return out_jobs

    def o_prod(s, j, m, n):
        i = (0, 1, 5, 6, 2, 3, 4)[n - 1]
        left = _side_by_side(*[cs[s, g, i, :, m * 128:(m + 1) * 128] for g in range(2)])
        if n in (2, 5):
            right = [wob[g, j, n // 5, n // 5] for g in range(2)]
        else:
            right = [wos[g, j, {1: 0, 3: 1, 4: 2, 6: 3, 7: 4}[n]] for g in range(2)]
        return _mm(left, jnp.concatenate(right, axis=0))

    def o_block(s, j, m, put):
        needs = [("c", s, m, g, p) for g in range(2) for p in all4]
        needs += [("wo", j, p) for p in all4] + [("wos", g, j, p) for g in range(2) for p in all4]
        return _strassen(lambda n: o_prod(s, j, m, n), put, needs)

    def finish(j, m, q, y):
        y = (y + rbuf[j, m, q].astype(F32)).astype(out.dtype)
        r, c = divmod(q, 2)
        for u in range(2):
            r0 = (4 * (2 * r + u) + m) * 64
            out[0, r0:r0 + 64, j * 256 + c * 128:j * 256 + (c + 1) * 128] = y[u * 64:(u + 1) * 64]

    def o_own(j, m):
        return o_block(0, j, m, lambda q, y: finish(j, m, q, y))

    def o_peer(j, m):
        def put(q, y):
            sbuf[j, m, q] = y
        return o_block(1, j, m, put)

    carried = []

    def run(*lists, flush=False):
        order = carried + _interleave(done, lists)
        quiet = [n + 1 for n, job in enumerate(order) if job.quiet]
        stop = quiet[-1] if quiet and not flush else len(order)
        for job in order[:stop]:
            job.fn(*job.args)
        carried[:] = order[stop:]

    def grid(s, ms, g, js):
        return [(s, m, g, j) for m in ms for j in js]

    def cast_x(m, kc):
        xb[0, m, kc] = xf[m, :, :, kc * 128:(kc + 1) * 128].reshape(256, 128)

    def cast_wq(j, kc):
        for e in range(2):
            wqb[0, j, kc, e] = wqf[j, kc * 128:(kc + 1) * 128, e * 128:(e + 1) * 128] * QSCALE

    for part in range(2):
        x_load(0, part).start()
        wq_load(0, part).start()
    for part in range(2):
        x_load(0, part).wait()
        wq_load(0, part).wait()
        (x_load, wq_load)[part](1).start()
        run([_Job(fn, (0, 4 * part + k)) for k in all4 for fn in (cast_x, cast_wq)], flush=True)
        if part == 0:
            pl.semaphore_wait(barrier, 2)
        start(send_x, 0, pl.ds(4 * part, 4))
        start(send_wq, 0, pl.ds(4 * part, 4))
    run(x_sums(0, 0) + wq_sums(0, 0) + q_proj([(0, 0, 0, 0)]))
    work = []
    for t in (1, 2, 3):
        x_load(t).wait()
        if t < 3:
            x_load(t + 1).start()
        else:
            kv_start(0, 0)
        run(work, [_Job(cast_x, (t, kc)) for kc in range(8)] + x_sums(0, t), flush=True)
        start(send_x, t)
        blocks = q_proj(grid(0, [t], 0, range(t)))
        keep = max(len(blocks) - KEEP, 0)
        run(blocks[:keep])
        wq_load(t).wait()
        if t < 3:
            wq_load(t + 1).start()
        else:
            kv_start(0, 1)
        run(blocks[keep:], [_Job(cast_wq, (t, kc)) for kc in range(8)] + wq_sums(0, t), flush=True)
        start(send_wq, t)
        blocks = q_proj(grid(0, range(t + 1), 0, [t]))
        keep = 14 if t == 3 else KEEP
        run(blocks[:-keep])
        work = blocks[-keep:]

    def got(t):
        recv(send_x, t)
        recv(send_wq, t)
        done.update([("x", 1, t), ("wq", 1, t)])

    def early(js, share):
        return js + [_Job(lambda: None, cost=len(js) * (1 / share - 1))]

    new1 = [(1, 1, 1, 0), (1, 0, 1, 1), (1, 1, 1, 1)]
    new2 = grid(1, [0, 1], 1, [2]) + grid(1, [2], 1, [0, 1, 2])
    new3 = grid(1, [0, 1, 2], 1, [3]) + grid(1, [3], 1, all4) + grid(1, [3], 0, all4)
    own = [(0, m, 1, j) for j in all4 for m in all4]

    run(work[:-7])
    kv_wait(0, 0, 0)
    run(work[-7:], attn(grid(0, [0], 0, [0, 1])))
    kv_wait(0, 0, 1)
    run(attn(grid(0, [0], 0, [2, 3])))
    kv_start(1, 0)
    got(0)
    run(q_proj(grid(1, [0], 0, all4)), x_sums(1, 0) + wq_sums(1, 0))
    kv_start(1, 1)
    kv_wait(0, 1)
    run(q_proj([(1, 0, 1, 0)] + own[:4]), attn(grid(1, [0], 0, all4) + grid(0, [1], 0, all4)))
    wo_load(0).start()
    kv_start(0, 2)
    got(1)
    run(q_proj(grid(1, [1], 0, all4) + new1 + own[4:5]), attn(grid(1, [1], 0, all4)),
        early(x_sums(1, 1) + wq_sums(1, 1), 0.4))
    wo_load(1).start()
    kv_start(1, 2)
    kv_wait(1, 0)
    kv_wait(1, 1)
    kv_wait(0, 2)
    run(q_proj(own[5:8]), attn([(1, 0, 1, 0)] + new1 + grid(0, [2], 0, all4)))
    kv_start(0, 3)
    kv_start(1, 3)
    wo_load(2).start()
    wo_load(3).start()
    wo_load(0).wait()
    got(2)
    run(q_proj(grid(1, [2], 0, all4) + new2 + own[8:8 + 1]), attn(grid(1, [2], 0, all4) + new2[:2]),
        early(x_sums(1, 2) + wq_sums(1, 2) + wo_cast(0), 0.8))
    start(send_wo, 0)
    kv_wait(1, 2)
    wo_load(1).wait()
    run(q_proj(own[8 + 1:11]), attn(new2[2:] + own[:2]), early(wo_cast(1), 0.7))
    start(send_wo, 1)
    kv_wait(0, 3)
    kv_wait(1, 3)
    got(3)
    run(q_proj(own[11:11 + 1] + new3), attn(new3), early(wq_sums(1, 3) + x_sums(1, 3), 0.4) + wo_sums(0))
    for j in (2, 3):
        wo_load(j).wait()

    mine = [o_own(j, m) for j in all4 for m in all4]

    def peer_rows(j):
        jobs = []
        for m in all4:
            block = o_peer(j, m)
            jobs += block[:1] + [_Job(start, (send_part, j, m - 1), cost=0)] * (m > 0) + block[1:]
        return jobs

    def send_last(j, jobs):
        return jobs[:1] + [_Job(start, (send_part, j, 3), cost=0)] + jobs[1:]

    def got_wo(j):
        recv(send_wo, j)
        return wo_sums(j, 1)

    run(q_proj(own[12:13]) + peer_rows(0), early(got_wo(0), 0.3) + early(wo_cast(2), 0.5))
    start(send_wo, 2)
    run(send_last(0, q_proj(own[13:15])), attn(grid(0, [3], 0, all4) + own[2:7]), early(wo_cast(3) + wo_sums(1), 0.75))
    start(send_wo, 3)
    run(q_proj(own[15:]) + peer_rows(1), early(got_wo(1), 0.25) + wo_sums(2))
    run(send_last(1, attn(own[7:])))
    recv(send_chunk, 0)
    run(mine[0], wo_sums(3))
    run(mine[1] + peer_rows(2), got_wo(2))
    run(send_last(2, mine[2] + mine[3]))
    recv(send_chunk, 1)
    run(sum(mine[4:6], []))
    run(mine[6] + peer_rows(3), got_wo(3))
    for t in all4:
        send_x(t).wait_send()
        send_wq(t).wait_send()
        send_wo(t).wait_send()
    run(send_last(3, sum(mine[6 + 1:8], [])))
    recv(send_chunk, 2)
    run(sum(mine[8:12], []))
    for m in range(3):
        recv(send_part, 3, m)
        run(mine[12 + m])
    last = []
    run(o_block(0, 3, 3, lambda q, y: last.append((q, y))), flush=True)
    recv(send_part, 3, 3)
    for q, y in last:
        finish(3, 3, q, y)
    remote(sbuf.refs, sbuf.refs, tx_p, rx_p.at[0], row_peer).wait_send()


def pallas_dist_sparse_attn_strided_qseq_b1_sq1024_skv1024_hq8_dh128_kernel(x, Wq, K_ext, V_ext, Wo):
    hbm = pl.BlockSpec(memory_space=pltpu.HBM)
    dma = pltpu.SemaphoreType.DMA
    return pl.pallas_call(
        _body,
        out_shape=jax.ShapeDtypeStruct((1, 1024, 1024), BF16),
        in_specs=[hbm] * 5,
        out_specs=pl.BlockSpec(memory_space=pltpu.VMEM),
        scratch_shapes=[
            pltpu.VMEM((4, 4, 64, 1024), F32), pltpu.VMEM((4, 1024, 256), F32), pltpu.VMEM((4, 1024, 256), F32),
            pltpu.VMEM((2, 4, 8, 2, 4, 64, 128), F32),
            _buffers((2, 4), (8, 256, 128), BF16), _buffers((2, 4), (4, 5, 128, 128), BF16),
            _buffers((2, 4), (8, 2, 128, 128), BF16), _buffers((2, 4), (4, 5, 128, 128), BF16),
            _buffers((2, 4), (2, 2, 512, 128), BF16), _buffers((2, 4), (5, 512, 128), BF16),
            _buffers((2, 4, 2, 4), (2, 256, 128), BF16), _buffers((2, 2), (7, 4, 512, 128), BF16),
            pltpu.VMEM((4, 4, 4, 128, 128), BF16), _buffers((4,), (4, 4, 128, 128), BF16),
            dma((5,)), dma((5,)), dma((4,)), dma((2, 5)),
            dma((4,)), dma((4,)), dma((4,)), dma((4,)), dma((4,)), dma((4,)), dma, dma((7,)),
        ],
        compiler_params=pltpu.CompilerParams(collective_id=0, vmem_limit_bytes=110 << 20),
    )(x.reshape(4, 4, 64, 1024), Wq, K_ext.reshape(4, 4, 64, 32, 128), V_ext.reshape(4, 4, 64, 32, 128), Wo)
```

```python
import jax
import jax.numpy as jnp
from jax import lax
from jax.experimental import pallas as pl
from jax.experimental.pallas import tpu as pltpu

F32, BF16 = jnp.float32, jnp.bfloat16
QSCALE = 0.08838834764831843 * 1.4426950408889634
LOOK = 7
STRIP = 64
KEEP = 2


class _Job:
    def __init__(self, fn, args=(), needs=(), gives=(), cost=1.0, quiet=False):
        self.fn, self.args, self.needs, self.gives, self.cost = fn, args, set(needs), set(gives), cost
        self.quiet = quiet


def _interleave(done, lists):
    lists = [list(js) for js in lists if js]
    total = [sum(j.cost for j in js) for js in lists]
    spent = [0.0] * len(lists)
    order = []
    while any(lists):
        ready = [n for n, js in enumerate(lists) if js and js[0].needs <= done]
        assert ready, [js[0].needs - done for js in lists if js]
        n = min(ready, key=lambda n: (spent[n] + lists[n][0].cost / 2) / total[n])
        job = lists[n].pop(0)
        spent[n] += job.cost
        done |= job.gives
        order.append(job)
    return order


def _lhs_sums(a11, a12, a21, a22):
    return a11 + a22, a21 + a22, a11 + a12, a21 - a11, a12 - a22


def _rhs_sums(b11, b12, b21, b22):
    return b11 + b22, b12 - b22, b21 - b11, b11 + b12, b21 + b22


def _mm(a, b):
    return jnp.dot(a, b, preferred_element_type=F32)


class _Packed:
    def __init__(self, refs):
        self.refs = refs

    def _pick(self, idx):
        ref = self.refs
        while isinstance(ref, (list, tuple)):
            ref, idx = ref[idx[0]], idx[1:]
        return ref, idx + (slice(None),) * (len(ref.shape) - len(idx))

    def __getitem__(self, idx):
        ref, idx = self._pick(idx)
        r = idx[-2]
        idx = idx[:-2] + (slice(None) if r.stop is None else slice(r.start // 2, r.stop // 2), idx[-1])
        return pltpu.bitcast(ref.bitcast(jnp.uint32)[idx], BF16)

    def __setitem__(self, idx, value):
        ref, idx = self._pick(idx)
        ref[idx] = value.astype(BF16)


def _buffers(lead, shape, dtype):
    if not lead:
        return pltpu.VMEM(shape, dtype)
    return [_buffers(lead[1:], shape, dtype) for _ in range(lead[0])]


def _wide(buf, idx, blocks, rows=slice(None)):
    return jnp.concatenate([buf[(*idx, k, rows)] for k in blocks], axis=1)


def _side_by_side(*stacks):
    tall = [stack.reshape(512, 128) for stack in stacks]
    return lax.concatenate([lax.slice_in_dim(t, k * 128, (k + 1) * 128) for t in tall for k in range(4)], 1)


def _strassen(product, put, needs, gives=()):
    m = {}

    def step(n):
        y = product(n)
        if n == 2:
            m["22"] = y
        elif n == 4:
            put(2, m["22"] + y)
            m["11"] = y
        elif n == 3:
            m["12"] = y
            m["22"] = y - m["22"]
        elif n == 5:
            put(1, m.pop("12") + y)
            m["11"] = m["11"] - y
        elif n == 1:
            m["11"], m["22"] = m["11"] + y, m["22"] + y
        elif n == 7:
            put(0, m.pop("11") + y)
        else:
            put(3, m.pop("22") + y)

    return [_Job(step, (n,), needs if n == 2 else (), gives if n == 6 else (), quiet=n < 4)
            for n in (2, 4, 3, 5, 1, 7, 6)]


def _body(x_hbm, wq_hbm, k_hbm, v_hbm, wo_hbm, out,
          xf, wqf, wof, kvf, xb, xs, wqb, wqs, wob, wos, qb, cs, sbuf, rbuf,
          x_sem, wq_sem, wo_sem, kv_sem, tx_x, rx_x, tx_q, rx_q, tx_o, rx_o, tx_p, rx_p):
    me = lax.axis_index("i")
    row_peer = me ^ 1
    head_peer = 3 - me
    mesh_id = pl.DeviceIdType.MESH
    lo, hi = slice(0, 512), slice(512, 1024)
    all4 = range(4)
    done = {("x", 0, m) for m in all4} | {("wq", 0, j) for j in all4}
    xb, xs, wqb, wqs, wob, wos, qb, cs, sbuf, rbuf = map(
        _Packed, (xb, xs, wqb, wqs, wob, wos, qb, cs, sbuf, rbuf))

    barrier = pltpu.get_barrier_semaphore()
    for peer in (row_peer, head_peer):
        pl.semaphore_signal(barrier, inc=1, device_id=(peer,), device_id_type=mesh_id)

    halves = (pl.ds(0, 512), pl.ds(512, 512), slice(None))

    def x_load(m, part=2):
        c = halves[part]
        return pltpu.make_async_copy(x_hbm.at[:, m, :, c], xf.at[m, :, :, c], x_sem.at[m + (part > 0)])

    def wq_load(j, part=2):
        r = halves[part]
        return pltpu.make_async_copy(wq_hbm.at[r, pl.ds(j * 256, 256)], wqf.at[j, r], wq_sem.at[j + (part > 0)])

    def wo_load(j):
        return pltpu.make_async_copy(wo_hbm.at[:, pl.ds(j * 256, 256)], wof.at[j], wo_sem.at[j])

    def kv_start(g, m):
        head0 = (me if g == 0 else head_peer) * 8
        for h in range(8):
            sem = kv_sem.at[0, 4] if (g, m) == (0, 0) and h >= 4 else kv_sem.at[g, m]
            for t, src in enumerate((k_hbm, v_hbm)):
                pltpu.make_async_copy(src.at[:, m, :, head0 + h, :], kvf.at[g, m, h, t], sem).start()

    def kv_wait(g, m, half=None):
        heads = slice(None) if half is None else pl.ds(4 * half, 4)
        sem = kv_sem.at[0, 4] if half else kv_sem.at[g, m]
        pltpu.make_async_copy(kvf.at[g, m, heads], kvf.at[g, m, heads], sem).wait()
        done.update(("kv", g, m, j) for j in all4 if half is None or j // 2 == half)

    def remote(src, dst, tx, rx, peer):
        return pltpu.make_async_remote_copy(src, dst, tx, rx, device_id=(peer,), device_id_type=mesh_id)

    def send_x(m, c=slice(None)):
        return remote(xb.refs[0][m].at[c], xb.refs[1][m].at[c], tx_x.at[m], rx_x.at[m], row_peer)

    def send_wq(j, r=slice(None)):
        return remote(wqb.refs[0][j].at[r], wqb.refs[1][j].at[r], tx_q.at[j], rx_q.at[j], head_peer)

    def send_wo(j):
        return remote(wob.refs[0][j], wob.refs[1][j], tx_o.at[j], rx_o.at[j], head_peer)

    def send_part(j, m):
        rx = rx_p.at[j + (m if j == 3 else 0)]
        return remote(sbuf.refs.at[j, m], rbuf.refs[j].at[m], tx_p, rx, row_peer)

    def send_chunk(j):
        return remote(sbuf.refs.at[j], rbuf.refs[j], tx_p, rx_p.at[j], row_peer)

    def start(make, *args):
        assert not any(job.fn is cast_wo for job in carried)
        make(*args).start()

    def recv(make, *args):
        make(*args).wait_recv()

    def strips(fn, items, needs, gives):
        rows = [slice(u * STRIP, (u + 1) * STRIP) for u in range(128 // STRIP)]
        return [_Job(fn, (*it, r), needs(*it), gives(*it) if r is rows[-1] else ()) for it in items for r in rows]

    def sum_x(s, m, k, r):
        if s == 0:
            a, t = divmod(r.start, 64)
            quads = [xf[m, 2 * e + a, t:t + STRIP, kk * 128:(kk + 1) * 128] for e in range(2) for kk in (k, k + 4)]
        else:
            quads = [xb[s, m, kk, e * 128 + r.start:e * 128 + r.stop].astype(F32) for e in range(2) for kk in (k, k + 4)]
        for i, v in enumerate(_lhs_sums(*quads)):
            xs[s, m, k, i, r] = v

    def x_sums(s, m):
        return strips(sum_x, [(s, m, k) for k in all4], lambda s, m, k: [("x", s, m)], lambda *it: [("xs", *it)])

    def sum_wq(g, j, k, r):
        if g == 0:
            quads = [wqf[j, kk * 128 + r.start:kk * 128 + r.stop, c * 128:(c + 1) * 128] * QSCALE
                     for kk in (k, k + 4) for c in range(2)]
        else:
            quads = [wqb[g, j, kk, c, r].astype(F32) for kk in (k, k + 4) for c in range(2)]
        for i, v in enumerate(_rhs_sums(*quads)):
            wqs[g, j, k, i, r] = v

    def wq_sums(g, j):
        return strips(sum_wq, [(g, j, k) for k in all4], lambda g, j, k: [("wq", g, j)], lambda *it: [("wqs", *it)])

    def wo_quads(j, p, r):
        return [wof[j, (2 * p + e) * 128 + r.start:(2 * p + e) * 128 + r.stop, c * 128:(c + 1) * 128]
                for e in range(2) for c in range(2)]

    def cast_wo(j, p, r):
        for n, v in enumerate(wo_quads(j, p, r)):
            wob[0, j, n % 2, n // 2, p * 128 + r.start:p * 128 + r.stop] = v

    def sum_wo(g, j, p, r):
        rows = slice(p * 128 + r.start, p * 128 + r.stop)
        quads = wo_quads(j, p, r) if g == 0 else [wob[g, j, c, e, rows].astype(F32) for e in range(2) for c in range(2)]
        for i, v in enumerate(_rhs_sums(*quads)):
            wos[g, j, i, rows] = v

    def wo_cast(j):
        return strips(cast_wo, [(j, p) for p in all4], lambda *it: (), lambda *it: [("wo", *it)])

    def wo_sums(j, g=0):
        return strips(sum_wo, [(g, j, p) for p in all4], lambda *it: (), lambda *it: [("wos", *it)])

    def q_block(s, m, g, j):
        def product(n):
            if n in (3, 4):
                left = xb[s, m, 4 * (n - 3):4 * (n - 2), (n - 3) * 128:(n - 2) * 128]
            else:
                left = xs[s, m, :, {1: 0, 2: 1, 5: 2, 6: 3, 7: 4}[n]]
            if n in (2, 5):
                right = wqb[g, j, 4 * (n // 5):4 * (n // 5) + 4, n // 5]
            else:
                right = wqs[g, j, :, {1: 0, 3: 1, 4: 2, 6: 3, 7: 4}[n]]
            return _mm(_side_by_side(left), right.reshape(512, 128))

        def put(q, y):
            qb[s, m, g, j, q % 2, q // 2 * 128:(q // 2 + 1) * 128] = y

        needs = [("xs", s, m, k) for k in all4] + [("wqs", g, j, k) for k in all4]
        return _strassen(product, put, needs, [("q", s, m, g, j)])

    def q_proj(items):
        return [job for it in items for job in q_block(*it)]

    def attn(pairs):
        items = [(s, m, g, j, r, e) for s, m, g, j in pairs for r, e in ((0, 0), (1, 1), (0, 1), (1, 0))]
        live = {}

        def scores(n):
            s, m, g, j, r, e = items[n]
            q = qb[s, m, g, j, e, r * 128:(r + 1) * 128, :]
            k = kvf[g, m, 2 * j + e, 0].reshape(256, 128).astype(BF16)
            sc = lax.dot_general(q, k, (((1,), (1,)), ((), ())), preferred_element_type=F32)
            p = jnp.exp2(sc - jnp.max(sc, axis=1, keepdims=True))
            live[n] = (p.astype(BF16), jnp.sum(p, axis=1, keepdims=True))

        def context(n):
            s, m, g, j, r, e = items[n]
            p, l = live.pop(n)
            v = kvf[g, m, 2 * j + e, 1].reshape(256, 128).astype(BF16)
            inv = pl.reciprocal(l, approx=True)
            o = _mm(p, v) * (inv * (2.0 - l * inv))

            def put(i, value):
                cs[s, g, i, j, m * 128:(m + 1) * 128, :] = value

            if (r, e) == (0, 0):
                live["11"] = o
                put(5, o)
            elif (r, e) == (1, 1):
                live["22"] = o
                put(6, o)
                put(0, live["11"] + o)
            elif (r, e) == (0, 1):
                put(2, live["11"] + o)
                put(4, o - live["22"])
            else:
                put(3, o - live.pop("11"))
                put(1, o + live.pop("22"))

        out_jobs = []
        for n in range(len(items) + LOOK):
            if n < len(items):
                s, m, g, j = items[n][:4]
                out_jobs.append(_Job(scores, (n,), [("q", s, m, g, j), ("kv", g, m, j)]))
            if n >= LOOK:
                last = (n - LOOK) % 4 == 3
                out_jobs.append(_Job(context, (n - LOOK,), (), [("c",) + items[n - LOOK][:4]] * last))
        return out_jobs

    def o_prod(s, j, m, n):
        i = (0, 1, 5, 6, 2, 3, 4)[n - 1]
        left = _side_by_side(*[cs[s, g, i, :, m * 128:(m + 1) * 128] for g in range(2)])
        if n in (2, 5):
            right = [wob[g, j, n // 5, n // 5] for g in range(2)]
        else:
            right = [wos[g, j, {1: 0, 3: 1, 4: 2, 6: 3, 7: 4}[n]] for g in range(2)]
        return _mm(left, jnp.concatenate(right, axis=0))

    def o_block(s, j, m, put):
        needs = [("c", s, m, g, p) for g in range(2) for p in all4]
        needs += [("wo", j, p) for p in all4] + [("wos", g, j, p) for g in range(2) for p in all4]
        return _strassen(lambda n: o_prod(s, j, m, n), put, needs)

    def finish(j, m, q, y):
        y = (y + rbuf[j, m, q].astype(F32)).astype(out.dtype)
        r, c = divmod(q, 2)
        for u in range(2):
            r0 = (4 * (2 * r + u) + m) * 64
            out[0, r0:r0 + 64, j * 256 + c * 128:j * 256 + (c + 1) * 128] = y[u * 64:(u + 1) * 64]

    def o_own(j, m):
        return o_block(0, j, m, lambda q, y: finish(j, m, q, y))

    def o_peer(j, m):
        def put(q, y):
            sbuf[j, m, q] = y
        return o_block(1, j, m, put)

    carried = []

    def run(*lists, flush=False):
        order = carried + _interleave(done, lists)
        quiet = [n + 1 for n, job in enumerate(order) if job.quiet]
        stop = quiet[-1] if quiet and not flush else len(order)
        for job in order[:stop]:
            job.fn(*job.args)
        carried[:] = order[stop:]

    def grid(s, ms, g, js):
        return [(s, m, g, j) for m in ms for j in js]

    def cast_x(m, kc):
        xb[0, m, kc] = xf[m, :, :, kc * 128:(kc + 1) * 128].reshape(256, 128)

    def cast_wq(j, kc):
        for e in range(2):
            wqb[0, j, kc, e] = wqf[j, kc * 128:(kc + 1) * 128, e * 128:(e + 1) * 128] * QSCALE

    for part in range(2):
        x_load(0, part).start()
        wq_load(0, part).start()
    for part in range(2):
        x_load(0, part).wait()
        wq_load(0, part).wait()
        (x_load, wq_load)[part](1).start()
        run([_Job(fn, (0, 4 * part + k)) for k in all4 for fn in (cast_x, cast_wq)], flush=True)
        if part == 0:
            pl.semaphore_wait(barrier, 2)
        start(send_x, 0, pl.ds(4 * part, 4))
        start(send_wq, 0, pl.ds(4 * part, 4))
    run(x_sums(0, 0) + wq_sums(0, 0) + q_proj([(0, 0, 0, 0)]))
    work = []
    for t in (1, 2, 3):
        x_load(t).wait()
        if t < 3:
            x_load(t + 1).start()
        else:
            kv_start(0, 0)
        run(work, [_Job(cast_x, (t, kc)) for kc in range(8)] + x_sums(0, t), flush=True)
        start(send_x, t)
        blocks = q_proj(grid(0, [t], 0, range(t)))
        keep = max(len(blocks) - KEEP, 0)
        run(blocks[:keep])
        wq_load(t).wait()
        if t < 3:
            wq_load(t + 1).start()
        else:
            kv_start(0, 1)
        run(blocks[keep:], [_Job(cast_wq, (t, kc)) for kc in range(8)] + wq_sums(0, t), flush=True)
        start(send_wq, t)
        blocks = q_proj(grid(0, range(t + 1), 0, [t]))
        keep = 14 if t == 3 else KEEP
        run(blocks[:-keep])
        work = blocks[-keep:]

    def got(t):
        recv(send_x, t)
        recv(send_wq, t)
        done.update([("x", 1, t), ("wq", 1, t)])

    def early(js, share):
        return js + [_Job(lambda: None, cost=len(js) * (1 / share - 1))]

    new1 = [(1, 1, 1, 0), (1, 0, 1, 1), (1, 1, 1, 1)]
    new2 = grid(1, [0, 1], 1, [2]) + grid(1, [2], 1, [0, 1, 2])
    new3 = grid(1, [0, 1, 2], 1, [3]) + grid(1, [3], 1, all4) + grid(1, [3], 0, all4)
    own = [(0, m, 1, j) for j in all4 for m in all4]

    run(work[:-7])
    kv_wait(0, 0, 0)
    run(work[-7:], attn(grid(0, [0], 0, [0, 1])))
    kv_wait(0, 0, 1)
    run(attn(grid(0, [0], 0, [2, 3])))
    kv_start(1, 0)
    got(0)
    run(q_proj(grid(1, [0], 0, all4)), x_sums(1, 0) + wq_sums(1, 0))
    kv_start(1, 1)
    kv_wait(0, 1)
    run(q_proj([(1, 0, 1, 0)] + own[:4]), attn(grid(1, [0], 0, all4) + grid(0, [1], 0, all4)))
    wo_load(0).start()
    kv_start(0, 2)
    kv_wait(1, 0)
    run(attn([(1, 0, 1, 0)] + own[:1]))
    got(1)
    run(q_proj(grid(1, [1], 0, all4) + new1 + own[4:5]), attn(grid(1, [1], 0, all4)),
        early(x_sums(1, 1) + wq_sums(1, 1), 0.4))
    wo_load(1).start()
    kv_start(1, 2)
    kv_wait(1, 1)
    kv_wait(0, 2)
    run(q_proj(own[5:8]), attn(new1 + grid(0, [2], 0, all4)))
    kv_start(0, 3)
    kv_start(1, 3)
    wo_load(2).start()
    wo_load(3).start()
    wo_load(0).wait()
    got(2)
    run(q_proj(grid(1, [2], 0, all4) + new2 + own[8:8 + 1]), attn(grid(1, [2], 0, all4) + new2[:2]),
        early(x_sums(1, 2) + wq_sums(1, 2) + wo_cast(0), 0.8))
    start(send_wo, 0)
    kv_wait(1, 2)
    wo_load(1).wait()
    run(q_proj(own[8 + 1:11]), attn(new2[2:] + own[1:2]), early(wo_cast(1), 0.7))
    start(send_wo, 1)
    kv_wait(0, 3)
    kv_wait(1, 3)
    got(3)
    run(q_proj(own[11:11 + 1] + new3), attn(new3), early(wq_sums(1, 3) + x_sums(1, 3), 0.4) + wo_sums(0))
    for j in (2, 3):
        wo_load(j).wait()

    mine = [o_own(j, m) for j in all4 for m in all4]

    def peer_rows(j):
        jobs = []
        for m in all4:
            block = o_peer(j, m)
            jobs += block[:1] + [_Job(start, (send_part, j, m - 1), cost=0)] * (m > 0) + block[1:]
        return jobs

    def send_last(j, jobs):
        return jobs[:1] + [_Job(start, (send_part, j, 3), cost=0)] + jobs[1:]

    def got_wo(j):
        recv(send_wo, j)
        return wo_sums(j, 1)

    run(q_proj(own[12:13]) + peer_rows(0), early(got_wo(0), 0.3) + early(wo_cast(2), 0.5))
    start(send_wo, 2)
    run(send_last(0, q_proj(own[13:15])), attn(grid(0, [3], 0, all4) + own[2:8]), early(wo_cast(3) + wo_sums(1), 0.75))
    start(send_wo, 3)
    run(q_proj(own[15:]) + peer_rows(1), early(got_wo(1), 0.25) + wo_sums(2))
    run(send_last(1, attn(own[8:])))
    recv(send_chunk, 0)
    run(mine[0] + mine[1][:4], wo_sums(3))
    run(mine[1][4:] + peer_rows(2), early(got_wo(2), 0.3))
    run(send_last(2, mine[2] + mine[3]))
    recv(send_chunk, 1)
    run(sum(mine[4:6], []))
    run(mine[6] + peer_rows(3), got_wo(3))
    for t in all4:
        send_x(t).wait_send()
        send_wq(t).wait_send()
        send_wo(t).wait_send()
    run(send_last(3, sum(mine[6 + 1:8], [])))
    recv(send_chunk, 2)
    run(sum(mine[8:12], []))
    for m in range(3):
        recv(send_part, 3, m)
        run(mine[12 + m])
    last = []
    run(o_block(0, 3, 3, lambda q, y: last.append((q, y))), flush=True)
    recv(send_part, 3, 3)
    for q, y in last:
        finish(3, 3, q, y)
    remote(sbuf.refs, sbuf.refs, tx_p, rx_p.at[0], row_peer).wait_send()


def pallas_dist_sparse_attn_strided_qseq_b1_sq1024_skv1024_hq8_dh128_kernel(x, Wq, K_ext, V_ext, Wo):
    hbm = pl.BlockSpec(memory_space=pltpu.HBM)
    dma = pltpu.SemaphoreType.DMA
    return pl.pallas_call(
        _body,
        out_shape=jax.ShapeDtypeStruct((1, 1024, 1024), BF16),
        in_specs=[hbm] * 5,
        out_specs=pl.BlockSpec(memory_space=pltpu.VMEM),
        scratch_shapes=[
            pltpu.VMEM((4, 4, 64, 1024), F32), pltpu.VMEM((4, 1024, 256), F32), pltpu.VMEM((4, 1024, 256), F32),
            pltpu.VMEM((2, 4, 8, 2, 4, 64, 128), F32),
            _buffers((2, 4), (8, 256, 128), BF16), _buffers((2, 4), (4, 5, 128, 128), BF16),
            _buffers((2, 4), (8, 2, 128, 128), BF16), _buffers((2, 4), (4, 5, 128, 128), BF16),
            _buffers((2, 4), (2, 2, 512, 128), BF16), _buffers((2, 4), (5, 512, 128), BF16),
            _buffers((2, 4, 2, 4), (2, 256, 128), BF16), _buffers((2, 2), (7, 4, 512, 128), BF16),
            pltpu.VMEM((4, 4, 4, 128, 128), BF16), _buffers((4,), (4, 4, 128, 128), BF16),
            dma((5,)), dma((5,)), dma((4,)), dma((2, 5)),
            dma((4,)), dma((4,)), dma((4,)), dma((4,)), dma((4,)), dma((4,)), dma, dma((7,)),
        ],
        compiler_params=pltpu.CompilerParams(collective_id=0, vmem_limit_bytes=110 << 20),
    )(x.reshape(4, 4, 64, 1024), Wq, K_ext.reshape(4, 4, 64, 32, 128), V_ext.reshape(4, 4, 64, 32, 128), Wo)
```
